```python
import numpy as np

kernel_name = "dist_rmsnorm_colshard_i_m768_n512"

def setup_inputs():
    x = np.random.randn(768, 2048).astype(np.float32)
    gamma = np.random.randn(2048).astype(np.float32)
    return {"x": x, "gamma": gamma}

def reference(x: np.ndarray, gamma: np.ndarray) -> np.ndarray:
    eps = 1e-5
    rms = np.sqrt(np.mean(x * x, axis=1, keepdims=True) + eps)
    return gamma * x / rms
```

```python
import jax, jax.numpy as jnp
from jax import lax
from jax.experimental import pallas as pl
from jax.experimental.pallas import tpu as pltpu
HBM = pl.BlockSpec(memory_space=pltpu.HBM)
def mk(chunks, p1="x", p2="x", nocheck=True, prio=None, inplace=False, flags=None, late_nbr=False, post=None, comm=True):
    starts = [sum(chunks[:i]) for i in range(len(chunks))]
    nb = [-(-c // 128) for c in chunks]
    K = len(chunks)
    def f(x, g):
        M, N = x.shape
        assert sum(chunks) == M
        def body(x_hbm, g_hbm, o_ref, xs, gbuf, ld, gsem, ss, rs, *cb):
            sb, rb = cb[:K], cb[K:]
            xbuf = o_ref if inplace else xs
            loads = [pltpu.make_async_copy(x_hbm.at[pl.ds(s, c)], xbuf.at[pl.ds(s, c)], ld.at[i]) for i, (s, c) in enumerate(zip(starts, chunks))]
            for i, c in enumerate(loads): c.start(**({} if prio is None else dict(priority=prio[i])))
            me = lax.axis_index("i")
            bar = pltpu.get_barrier_semaphore()
            for d in (2, 1, 3):
                pl.semaphore_signal(bar, 1, device_id=((me + d) % 4,), device_id_type=pl.DeviceIdType.MESH)
            gc = pltpu.make_async_copy(g_hbm, gbuf, gsem); gc.start()
            lane = lax.broadcasted_iota(jnp.int32, (8, 128), 1)
            sub = lax.broadcasted_iota(jnp.int32, (8, 128), 0)
            def rd(i, d):
                return pltpu.make_async_remote_copy(sb[i], rb[i].at[d - 1], ss.at[3 * i + d - 1], rs.at[i], device_id=((me + d) % 4,), device_id_type=pl.DeviceIdType.MESH)
            sends = []
            def sq(r0, n):
                v = xbuf[pl.ds(r0, n), :]; v = v * v
                return (v[:, 0:128] + v[:, 128:256]) + (v[:, 256:384] + v[:, 384:512])
            for i, (s, c) in enumerate(zip(starts, chunks)):
                loads[i].wait()
                m1 = p1[i] if len(p1) > 1 else p1
                for b in range(nb[i]):
                    n = min(128, c - 128 * b); r0 = s + 128 * b
                    if m1 == "x":
                        acc = jnp.zeros((8, 128), jnp.float32)
                        for j in range(n // 8):
                            red = jnp.sum(sq(r0 + 8 * j, 8), axis=1, keepdims=True)
                            acc = jnp.where(lane == sub + 8 * j, red, acc)
                        row = jnp.sum(acc, axis=0, keepdims=True)
                    else:
                        p = sq(r0, n)
                        if n < 128: p = jnp.concatenate([p, jnp.zeros((128 - n, 128), jnp.float32)], 0)
                        if m1 == "t": row = jnp.sum(p.T, axis=0, keepdims=True)
                        else: row = lax.dot_general(jnp.ones((8, 128), jnp.float32), p, (((1,), (1,)), ((), ())), preferred_element_type=jnp.float32)[0:1]
                    sb[i][pl.ds(b, 1), :] = row
                if i == 0: pl.semaphore_wait(bar, 3)
                if comm:
                    for d in ((2,) if late_nbr else (2, 1, 3)):
                        cp = rd(i, d); cp.start(); sends.append(cp)
            if late_nbr:
                for i in range(K):
                    for d in (1, 3):
                        cp = rd(i, d); cp.start(); sends.append(cp)
            gc.wait()
            gv = gbuf[...].reshape(1, N)
            for i, (s, c) in enumerate(zip(starts, chunks)):
                if i == K - 1:
                    for cp in sends: cp.wait_send()
                if comm: pltpu.make_async_copy(rb[i], rb[i], rs.at[i]).wait()
                m2 = p2[i] if len(p2) > 1 else p2
                for b in range(nb[i]):
                    n = min(128, c - 128 * b); r0 = s + 128 * b
                    q = pl.ds(b, 1)
                    tot = (sb[i][q, :] + rb[i][0, q, :]) + (rb[i][1, q, :] + rb[i][2, q, :])
                    r = lax.rsqrt(tot * (1.0 / (4 * N)) + 1e-5)
                    if m2 == "x":
                        r8 = jnp.broadcast_to(r, (8, 128))
                        for j in range(n // 8):
                            rj = jnp.sum(jnp.where(lane == sub + 8 * j, r8, 0.0), axis=1, keepdims=True)
                            rows = pl.ds(r0 + 8 * j, 8)
                            o_ref[rows, :] = ((xbuf[rows, :] * gv) * rj).astype(o_ref.dtype)
                    else:
                        rt = jnp.broadcast_to(r, (128, 128)).T[:n]
                        rows = pl.ds(r0, n)
                        o_ref[rows, :] = ((xbuf[rows, :] * gv) * jnp.concatenate([rt] * 4, axis=1)).astype(o_ref.dtype)
        kw = dict(disable_bounds_checks=True, disable_semaphore_checks=True) if nocheck else {}
        if flags: kw["flags"] = flags
        out = pl.pallas_call(body, out_shape=jax.ShapeDtypeStruct(x.shape, x.dtype), in_specs=[HBM, HBM], out_specs=pl.BlockSpec(memory_space=pltpu.VMEM),
            scratch_shapes=[pltpu.VMEM((8, 128) if inplace else x.shape, x.dtype), pltpu.VMEM((1, N), g.dtype), pltpu.SemaphoreType.DMA((K,)), pltpu.SemaphoreType.DMA,
                            pltpu.SemaphoreType.DMA((3 * K,)), pltpu.SemaphoreType.DMA((K,))]
                + [pltpu.VMEM((n, 128), jnp.float32) for n in nb] + [pltpu.VMEM((3, n, 128), jnp.float32) for n in nb],
            compiler_params=pltpu.CompilerParams(collective_id=0, **kw))(x, g.reshape(1, N))
        return out
    return f


def pallas_dist_rmsnorm_colshard_i_m768_n512_kernel(x, gamma):
    return mk((640, 128), "x", "x")(x, gamma)
```

```python
import jax
import jax.numpy as jnp
from jax import lax
from jax.experimental import pallas as pl
from jax.experimental.pallas import tpu as pltpu

_N_DEV = 4
_EPS = 1e-5
_SUB, _LANE = 8, 128

_PIECES = (256, 128, 128, 128, 80, 8, 32, 8)
_GROUPS = (384, 128, 128, 88, 40)


def _offsets(sizes):
    return [sum(sizes[:i]) for i in range(len(sizes) + 1)]


def pallas_dist_rmsnorm_colshard_i_m768_n512_kernel(
    x: jax.Array,
    gamma: jax.Array,
):
    m, n = x.shape
    n_total = _N_DEV * n
    piece_at, group_at = _offsets(_PIECES), _offsets(_GROUPS)
    n_groups = len(_GROUPS)
    assert piece_at[-1] == group_at[-1] == m and n % _LANE == 0

    wires = [
        (group_at[k] + o, min(_LANE, rows - o))
        for k, rows in enumerate(_GROUPS)
        for o in range(0, rows, _LANE)
    ]
    n_wires = len(wires)
    n_early = n_wires - (n_groups - 1)
    late_at = group_at[1]
    assert wires[n_early][0] == late_at
    assert all(r0 + rows in piece_at for r0, rows in wires[n_early - 1 :])

    def body(
        x_hbm, gamma_hbm, out_ref,
        x_buf, gamma_buf, mine, from_nbrs, early, late, late_base,
        load_sems, gamma_sem, send_sems, recv_sems,
    ):
        loads = [
            pltpu.make_async_copy(
                x_hbm.at[pl.ds(piece_at[i], rows)],
                x_buf.at[pl.ds(piece_at[i], rows)],
                load_sems.at[i],
            )
            for i, rows in enumerate(_PIECES)
        ]
        loads[0].start()

        me = lax.axis_index("i")

        def peer(d):
            return dict(
                device_id=((me + d) % _N_DEV,),
                device_id_type=pl.DeviceIdType.MESH,
            )

        barrier = pltpu.get_barrier_semaphore()
        for d in (2, 1, 3):
            pl.semaphore_signal(barrier, 1, **peer(d))
        for load in loads[1:]:
            load.start()

        routes = [(mine.at[pl.ds(0, n_early)], early)] + [
            (mine.at[n_early + k], late.at[k]) for k in range(n_groups - 1)
        ]
        to_diag = [
            pltpu.make_async_remote_copy(
                src, dst, send_sems.at[k], recv_sems.at[k], **peer(2)
            )
            for k, (src, dst) in enumerate(routes)
        ]
        to_nbrs = [
            pltpu.make_async_remote_copy(
                mine,
                from_nbrs.at[j],
                send_sems.at[n_groups + j],
                recv_sems.at[n_groups],
                **peer(d),
            )
            for j, d in enumerate((1, 3))
        ]

        sub = lax.broadcasted_iota(jnp.int32, (_SUB, _LANE), 0)
        lane = lax.broadcasted_iota(jnp.int32, (_SUB, _LANE), 1)
        diag = lane - sub

        for w, (r0, rows) in enumerate(wires):
            folded = []
            for r in range(r0, r0 + rows, _SUB):
                if r in piece_at:
                    loads[piece_at.index(r)].wait()
                v = x_buf[pl.ds(r, _SUB), :]
                v = v * v
                parts = [v[:, c : c + _LANE] for c in range(0, n, _LANE)]
                while len(parts) > 1:
                    parts = parts[2:] + [parts[0] + parts[1]]
                folded.append(parts[0])
            acc = jnp.zeros((_SUB, _LANE), jnp.float32)
            for j, f in enumerate(folded):
                total = jnp.sum(f, axis=1, keepdims=True)
                acc = jnp.where(diag == _SUB * j, total, acc)
            mine[w] = jnp.sum(acc, axis=0, keepdims=True)
            if r0 + rows in group_at:
                k = group_at.index(r0 + rows) - 1
                if k == 0:
                    pl.semaphore_wait(barrier, _N_DEV - 1)
                to_diag[k].start()
        for copy in to_nbrs:
            copy.start()

        gamma_load = pltpu.make_async_copy(gamma_hbm, gamma_buf, gamma_sem)
        gamma_load.start()
        gamma_load.wait()
        scale = gamma_buf[...] * float(n_total) ** 0.5
        for copy in to_diag + to_nbrs:
            copy.wait_send()
        pltpu.make_async_copy(from_nbrs, from_nbrs, recv_sems.at[n_groups]).wait()

        def near_sum(w):
            s = mine[w] + from_nbrs[0, w] + from_nbrs[1, w] + n_total * _EPS
            return jnp.broadcast_to(s, (_SUB, _LANE))

        def column(v, j):
            picked = jnp.where(diag == _SUB * j, v, 0.0)
            return jnp.sum(picked, axis=1, keepdims=True)

        for w in range(n_early, n_wires):
            r0, rows = wires[w]
            near = near_sum(w)
            for j in range(rows // _SUB):
                r = r0 + _SUB * j
                late_base[pl.ds(r - late_at, _SUB), :] = jnp.broadcast_to(
                    column(near, j), (_SUB, _LANE)
                )
                x_buf[pl.ds(r, _SUB), :] = x_buf[pl.ds(r, _SUB), :] * scale

        near = [near_sum(w) for w in range(n_early)]
        to_diag[0].wait_recv()
        for w in range(n_early):
            r0, rows = wires[w]
            inv = lax.rsqrt(jnp.broadcast_to(early[w], (_SUB, _LANE)) + near[w])
            for j in range(rows // _SUB):
                at = pl.ds(r0 + _SUB * j, _SUB)
                out_ref[at, :] = (x_buf[at, :] * scale) * column(inv, j)

        for k in range(n_groups - 1):
            r0, rows = wires[n_early + k]
            to_diag[k + 1].wait_recv()
            for q in range(0, rows, _SUB):
                far = [
                    jnp.full((_SUB, _LANE), late[k, 0, q + s], jnp.float32)
                    for s in range(_SUB)
                ]
                for bit in (1, 2, 4):
                    far = [
                        jnp.where((sub & bit) != 0, far[i + 1], far[i])
                        for i in range(0, len(far), 2)
                    ]
                base = late_base[pl.ds(r0 + q - late_at, _SUB), :]
                inv = lax.rsqrt(far[0] + base)
                at = pl.ds(r0 + q, _SUB)
                out_ref[at, :] = x_buf[at, :] * jnp.concatenate(
                    [inv] * (n // _LANE), axis=1
                )

    f32 = jnp.float32
    dma = pltpu.SemaphoreType.DMA
    hbm = pl.BlockSpec(memory_space=pltpu.HBM)
    return pl.pallas_call(
        body,
        out_shape=jax.ShapeDtypeStruct((m, n), f32),
        in_specs=[hbm, hbm],
        out_specs=pl.BlockSpec(memory_space=pltpu.VMEM),
        scratch_shapes=[
            pltpu.VMEM((m, n), f32),
            pltpu.VMEM((1, n), f32),
            pltpu.VMEM((n_wires, 1, _LANE), f32),
            pltpu.VMEM((2, n_wires, 1, _LANE), f32),
            pltpu.VMEM((n_early, 1, _LANE), f32),
            pltpu.SMEM((n_groups - 1, 1, _LANE), f32),
            pltpu.VMEM((m - late_at, _LANE), f32),
            dma((len(_PIECES),)),
            dma,
            dma((n_groups + 2,)),
            dma((n_groups + 1,)),
        ],
        compiler_params=pltpu.CompilerParams(
            collective_id=0,
            disable_semaphore_checks=True,
        ),
    )(x.astype(f32), gamma.astype(f32).reshape(1, n))
```
